```python
import numpy as np

kernel_name = "dist_argmax_global_i_m4096_n1024"

def setup_inputs():
    return {"x": np.random.randn(16384, 1024).astype(np.float32)}

def reference(x: np.ndarray) -> np.ndarray:
    idx = np.argmax(x, axis=0).astype(np.float32)
    val = np.max(x, axis=0)
    return np.stack([val, idx], axis=0)
```

```python
import jax
import jax.numpy as jnp
import numpy as np
from jax import lax
from jax.experimental import pallas as pl
from jax.experimental.pallas import tpu as pltpu

N_DEV = 4
I32_MIN = np.int32(-(2**31))
I32_MAX = np.int32(2**31 - 1)
MESH = pl.DeviceIdType.MESH


def _to_key(x):
    b = lax.bitcast_convert_type(x, jnp.int32)
    k = jnp.where(b < 0, I32_MIN - b, b)
    return jnp.where(x != x, I32_MAX, k)


def _from_key(k):
    return lax.bitcast_convert_type(jnp.where(k < 0, I32_MIN - k, k), jnp.float32)


def _better(k1, i1, k2, i2):
    take = jnp.logical_or(k2 > k1, jnp.logical_and(k2 == k1, i2 < i1))
    return jnp.where(take, k2, k1), jnp.where(take, i2, i1)


def _butterfly(ks, ids):
    sub = lax.broadcasted_iota(jnp.int32, (8, 128), 0)
    step = 4
    while len(ks) > 1:
        h = len(ks) // 2
        lo = (sub & step) == 0
        nk, ni = [], []
        for j in range(h):
            ak = jnp.where(lo, ks[j], pltpu.roll(ks[j + h], step, 0))
            ai = jnp.where(lo, ids[j], pltpu.roll(ids[j + h], step, 0))
            bk = jnp.where(lo, pltpu.roll(ks[j], 8 - step, 0), ks[j + h])
            bi = jnp.where(lo, pltpu.roll(ids[j], 8 - step, 0), ids[j + h])
            k, i = _better(ak, ai, bk, bi)
            nk.append(k)
            ni.append(i)
        ks, ids = nk, ni
        step //= 2
    return ks[0], ids[0]


def pallas_dist_argmax_global_i_m4096_n1024_kernel(x: jax.Array):
    rows, cols = x.shape
    chunks = [2048, 1024, 512, 256, 128, 64, 32, 32]
    assert sum(chunks) == rows and cols == 1024
    starts = np.cumsum([0] + chunks)[:-1].tolist()
    nc = len(chunks)
    unroll = 8

    def body(x_hbm, o_ref, xbuf, lsem, sbuf, rbuf, ssem, rsem):
        me = lax.axis_index("i")
        loads = [
            pltpu.make_async_copy(
                x_hbm.at[pl.ds(starts[c], chunks[c])],
                xbuf.at[pl.ds(starts[c], chunks[c])],
                lsem.at[c],
            )
            for c in range(nc)
        ]
        for ld in loads:
            ld.start()
        bar = pltpu.get_barrier_semaphore()
        offs = (2, 1, 3)
        peers = [(me + off) & (N_DEV - 1) for off in offs]
        for p in peers:
            pl.semaphore_signal(bar, inc=1, device_id=(p,), device_id_type=MESH)

        base = me * rows
        m = jnp.full((8, cols), I32_MIN, jnp.int32)
        idx = jnp.zeros((8, cols), jnp.int32) + base

        def step(r0, m, idx):
            k = _to_key(xbuf[pl.ds(r0, 8), :])
            take = k > m
            return jnp.where(take, k, m), jnp.where(take, r0 + base, idx)

        for c in range(nc):
            loads[c].wait()
            if c == 1:
                pl.semaphore_wait(bar, N_DEV - 1)
            ng = chunks[c] // 8
            u = min(unroll, ng)

            def loop_body(i, carry, c=c, u=u):
                m, idx = carry
                r = pl.multiple_of(starts[c] + i * (8 * u), 8)
                for j in range(u):
                    m, idx = step(r + 8 * j, m, idx)
                return m, idx

            if ng == u:
                m, idx = loop_body(0, (m, idx))
            else:
                m, idx = lax.fori_loop(0, ng // u, loop_body, (m, idx))

        idx = idx + lax.broadcasted_iota(jnp.int32, (8, cols), 0)
        k, i = _butterfly(
            [m[:, 128 * j : 128 * (j + 1)] for j in range(8)],
            [idx[:, 128 * j : 128 * (j + 1)] for j in range(8)],
        )
        sbuf[0:8, :] = k
        sbuf[8:16, :] = i
        sends = []
        for n, off in enumerate(offs):
            cp = pltpu.make_async_remote_copy(
                sbuf,
                rbuf.at[N_DEV - off - 1],
                ssem.at[n],
                rsem.at[N_DEV - off - 1],
                device_id=(peers[n],),
                device_id_type=MESH,
            )
            cp.start()
            sends.append(cp)
        for s in (0, 2, 1):
            pltpu.make_async_remote_copy(
                sbuf, rbuf.at[s], ssem.at[0], rsem.at[s],
                device_id=(me,), device_id_type=MESH,
            ).wait_recv()
            k, i = _better(k, i, rbuf[s, 0:8, :], rbuf[s, 8:16, :])
        val = _from_key(k)
        fi = i.astype(jnp.float32)
        for j in range(8):
            o_ref[0:1, 128 * j : 128 * (j + 1)] = pltpu.roll(val, (8 - j) % 8, 0)[0:1, :]
            o_ref[1:2, 128 * j : 128 * (j + 1)] = pltpu.roll(fi, (8 - j) % 8, 0)[0:1, :]
        for cp in sends:
            cp.wait_send()

    return pl.pallas_call(
        body,
        out_shape=jax.ShapeDtypeStruct((2, cols), jnp.float32),
        in_specs=[pl.BlockSpec(memory_space=pl.ANY)],
        out_specs=pl.BlockSpec(memory_space=pltpu.VMEM),
        scratch_shapes=[
            pltpu.VMEM((rows, cols), jnp.float32),
            pltpu.SemaphoreType.DMA((nc,)),
            pltpu.VMEM((16, 128), jnp.int32),
            pltpu.VMEM((3, 16, 128), jnp.int32),
            pltpu.SemaphoreType.DMA((3,)),
            pltpu.SemaphoreType.DMA((3,)),
        ],
        compiler_params=pltpu.CompilerParams(
            vmem_limit_bytes=40 * 1024 * 1024,
            collective_id=0,
            disable_semaphore_checks=True,
            disable_bounds_checks=True,
        ),
    )(x)
```

```python
import jax
import jax.numpy as jnp
import numpy as np
from jax import lax
from jax.experimental import pallas as pl
from jax.experimental.pallas import tpu as pltpu

N_DEV = 4
LANES = 128
SUBLANES = 8
I32_MIN = np.int32(-(2**31))
I32_MAX = np.int32(2**31 - 1)
MESH = pl.DeviceIdType.MESH


def _to_key(x):
  bits = lax.bitcast_convert_type(x, jnp.int32)
  key = jnp.where(bits < 0, I32_MIN - bits, bits)
  return jnp.where(x != x, I32_MAX, key)


def _from_key(key):
  bits = jnp.where(key < 0, I32_MIN - key, key)
  return lax.bitcast_convert_type(bits, jnp.float32)


def _better(a, b):
  (ka, ia), (kb, ib) = a, b
  take = jnp.logical_or(kb > ka, jnp.logical_and(kb == ka, ib < ia))
  return jnp.where(take, kb, ka), jnp.where(take, ib, ia)


def _sublane():
  return lax.broadcasted_iota(jnp.int32, (SUBLANES, LANES), 0)


def _fold4(keys, rows):
  sub = _sublane()
  pairs = list(zip(keys, rows))
  for step in (2, 1):
    half = len(pairs) // 2
    lo = (sub & step) == 0
    merged = []
    for j in range(half):
      p, q = pairs[j], pairs[j + half]
      a = tuple(jnp.where(lo, u, pltpu.roll(v, step, 0)) for u, v in zip(p, q))
      b = tuple(
          jnp.where(lo, pltpu.roll(u, SUBLANES - step, 0), v)
          for u, v in zip(p, q)
      )
      merged.append(_better(a, b))
    pairs = merged
  return _better(pairs[0], tuple(pltpu.roll(v, 4, 0) for v in pairs[0]))


def _build(rows, cols, chunks, tail, push, foreign_after, unroll=8, interpret=False):
  half = cols // 2
  local = rows - 2 * push
  tail_rows = sum(tail[0])
  assert cols == 8 * LANES and sum(tail[1]) == tail_rows
  assert sum(chunks) + tail_rows == local
  assert all(n % SUBLANES == 0 for n in (*chunks, *tail[0], *tail[1], push))
  chunk_start = np.cumsum([0, *chunks])[:-1].tolist()
  tail_start = [
      (local - tail_rows + np.cumsum([0, *t])[:-1]).tolist() for t in tail
  ]
  n_chunks = len(chunks)
  n_tail = (len(tail[0]), len(tail[1]))
  n_loads = n_chunks + sum(n_tail)
  send_order = ((2, 1), (1, 2), (3, 0))
  recv_order = (0, 2, 1)

  def body(x_hbm, out_ref, *scratch):
    scratch = list(scratch)
    chunk_buf = [scratch.pop(0) for _ in range(n_chunks)]
    tail_buf = [[scratch.pop(0) for _ in range(n)] for n in n_tail]
    from_left, from_right = scratch.pop(0), scratch.pop(0)
    (send_buf, recv_buf, load_sems, send_sems, recv_sems, push_send_sems,
     push_recv_sems) = scratch

    me = lax.axis_index("i")
    peer = {off: (me + off) & (N_DEV - 1) for off in (1, 2, 3)}
    right, left = peer[1], peer[3]

    chunk_copy = [
        pltpu.make_async_copy(
            x_hbm.at[pl.ds(chunk_start[c], chunks[c])],
            chunk_buf[c],
            load_sems.at[c],
        )
        for c in range(n_chunks)
    ]
    tail_copy = [
        [
            pltpu.make_async_copy(
                x_hbm.at[pl.ds(tail_start[h][c], tail[h][c]), pl.ds(h * half, half)],
                tail_buf[h][c],
                load_sems.at[n_chunks + h * n_tail[0] + c],
            )
            for c in range(n_tail[h])
        ]
        for h in range(2)
    ]
    for copy in chunk_copy + tail_copy[0] + tail_copy[1]:
      copy.start()

    barrier = pltpu.get_barrier_semaphore()
    for off in (1, 2, 3):
      pl.semaphore_signal(
          barrier, inc=1, device_id=(peer[off],), device_id_type=MESH
      )
    pl.semaphore_wait(barrier, N_DEV - 1)

    pushes = [
        pltpu.make_async_remote_copy(
            x_hbm.at[pl.ds(local, push)], from_left,
            push_send_sems.at[0], push_recv_sems.at[0],
            device_id=(right,), device_id_type=MESH,
        ),
        pltpu.make_async_remote_copy(
            x_hbm.at[pl.ds(local + push, push)], from_right,
            push_send_sems.at[1], push_recv_sems.at[1],
            device_id=(left,), device_id_type=MESH,
        ),
    ]
    for copy in pushes:
      copy.start()

    def fresh(width, first_row):
      return (
          jnp.full((SUBLANES, width), I32_MIN, jnp.int32),
          jnp.zeros((SUBLANES, width), jnp.int32) + first_row,
      )

    def scan(buf, first_row, state):
      groups = buf.shape[0] // SUBLANES
      u = min(unroll, groups)
      while groups % u:
        u -= 1

      def step(i, state):
        key, row = state
        r0 = pl.multiple_of(i * (SUBLANES * u), SUBLANES)
        for j in range(u):
          r = r0 + SUBLANES * j
          k = _to_key(buf[pl.ds(r, SUBLANES), :])
          take = k > key
          key = jnp.where(take, k, key)
          row = jnp.where(take, first_row + r, row)
        return key, row

      if groups == u:
        return step(0, state)
      return lax.fori_loop(0, groups // u, step, state)

    sub = _sublane()

    def fold(state, h):
      key, row = state
      g0 = 0 if key.shape[1] == half else h * half // LANES
      cut = lambda v, j: v[:, (g0 + j) * LANES:(g0 + j + 1) * LANES]
      return _fold4(
          [cut(key, j) for j in range(4)],
          [cut(row, j) + sub for j in range(4)],
      )

    my_row0 = me * rows
    state = fresh(cols, my_row0)
    for c in range(n_chunks):
      chunk_copy[c].wait()
      state = scan(chunk_buf[c], my_row0 + chunk_start[c], state)
      if c == foreign_after:
        pushes[0].wait_recv()
        row0 = left * rows + local
        got = scan(from_left, row0, fresh(cols, row0))
        foreign = [fold(got, h) for h in range(2)]
        pushes[1].wait_recv()
        row0 = right * rows + local + push
        got = scan(from_right, row0, fresh(cols, row0))
        foreign = [_better(foreign[h], fold(got, h)) for h in range(2)]

    sends, mine = [], []
    for h in range(2):
      part = tuple(v[:, h * half:(h + 1) * half] for v in state)
      for c in range(n_tail[h]):
        tail_copy[h][c].wait()
        part = scan(tail_buf[h][c], my_row0 + tail_start[h][c], part)
      key, row = _better(fold(part, h), foreign[h])
      message = jnp.where(sub < 4, key, row)
      send_buf[h] = message
      mine.append(message)
      for n, (off, slot) in enumerate(send_order):
        copy = pltpu.make_async_remote_copy(
            send_buf.at[h], recv_buf.at[h, slot],
            send_sems.at[h, n], recv_sems.at[h, slot],
            device_id=(peer[off],), device_id_type=MESH,
        )
        copy.start()
        sends.append(copy)

    for copy in pushes + sends:
      copy.wait_send()

    unpack = lambda m: (m, pltpu.roll(m, 4, 0))
    for h in range(2):
      best = unpack(mine[h])
      for slot in recv_order:
        pltpu.make_async_remote_copy(
            send_buf.at[h], recv_buf.at[h, slot],
            send_sems.at[h, 0], recv_sems.at[h, slot],
            device_id=(me,), device_id_type=MESH,
        ).wait_recv()
        best = _better(best, unpack(recv_buf[h, slot]))
      val, idx = _from_key(best[0]), best[1].astype(jnp.float32)
      for j in range(4):
        lanes = pl.ds((4 * h + j) * LANES, LANES)
        out_ref[0:1, lanes] = pltpu.roll(val, (SUBLANES - j) % SUBLANES, 0)[0:1]
        out_ref[1:2, lanes] = pltpu.roll(idx, (SUBLANES - j) % SUBLANES, 0)[0:1]

  def fn(x):
    assert x.shape == (rows, cols) and x.dtype == jnp.float32
    vmem = lambda shape, dtype=jnp.float32: pltpu.VMEM(shape, dtype)
    scratch_shapes = (
        [vmem((n, cols)) for n in chunks]
        + [vmem((n, half)) for t in tail for n in t]
        + [vmem((push, cols)), vmem((push, cols))]
        + [
            vmem((2, SUBLANES, LANES), jnp.int32),
            vmem((2, N_DEV - 1, SUBLANES, LANES), jnp.int32),
            pltpu.SemaphoreType.DMA((n_loads,)),
            pltpu.SemaphoreType.DMA((2, N_DEV - 1)),
            pltpu.SemaphoreType.DMA((2, N_DEV - 1)),
            pltpu.SemaphoreType.DMA((2,)),
            pltpu.SemaphoreType.DMA((2,)),
        ]
    )
    return pl.pallas_call(
        body,
        out_shape=jax.ShapeDtypeStruct((2, cols), jnp.float32),
        in_specs=[pl.BlockSpec(memory_space=pl.ANY)],
        out_specs=pl.BlockSpec(memory_space=pltpu.VMEM),
        scratch_shapes=scratch_shapes,
        compiler_params=pltpu.CompilerParams(
            collective_id=0,
            vmem_limit_bytes=32 * 1024 * 1024,
            disable_semaphore_checks=True,
        ),
        interpret=interpret,
    )(x)

  return fn


def pallas_dist_argmax_global_i_m4096_n1024_kernel(x: jax.Array):
  return _build(
      rows=4096,
      cols=1024,
      chunks=(2048, 1024, 256, 224),
      tail=((144,), (112, 32)),
      push=200,
      foreign_after=2,
  )(x)
```
